```python
import numpy as np

kernel_name = "dist_halo_stencil_i_m8192_n1024"

def setup_inputs():
    return {"x": np.random.randn(32768, 1024).astype(np.float32)}

def reference(x: np.ndarray) -> np.ndarray:
    out = np.empty_like(x)
    out[0] = x[0]
    out[-1] = x[-1]
    out[1:-1] = 0.25 * x[:-2] + 0.5 * x[1:-1] + 0.25 * x[2:]
    return out
```

```python
import jax
import jax.numpy as jnp
from jax import lax
from jax.experimental import pallas as pl
from jax.experimental.pallas import tpu as pltpu

AXIS = "i"
SUB = 8
TAIL = 64
STRIDE = 128


def pallas_dist_halo_stencil_i_m8192_n1024_kernel(x: jax.Array):
    m, n = x.shape
    half = m // 2

    def body(x_hbm, o_hbm, xb, ob, sem, halo_sem):
        def read(r0, rows, s):
            return pltpu.make_async_copy(
                x_hbm.at[pl.ds(r0, rows)], xb.at[pl.ds(SUB + r0, rows)], sem.at[s])

        rd_a, rd_b = read(0, half, 0), read(half, half - TAIL, 1)
        rd_a.start()
        rd_b.start()

        me = lax.axis_index(AXIS)
        has_l, has_r = me > 0, me < lax.axis_size(AXIS) - 1
        bar = pltpu.get_barrier_semaphore()

        @pl.when(has_l)
        def _():
            pl.semaphore_signal(bar, 1, device_id=(me - 1,), device_id_type=pl.DeviceIdType.MESH)

        @pl.when(has_r)
        def _():
            pl.semaphore_signal(bar, 1, device_id=(me + 1,), device_id_type=pl.DeviceIdType.MESH)

        sub = lax.broadcasted_iota(jnp.int32, (SUB, n), 0)

        def stencil(p, c, nx):
            up = pltpu.roll(jnp.where(sub == SUB - 1, p, c), 1, 0)
            dn = pltpu.roll(jnp.where(sub == 0, nx, c), SUB - 1, 0)
            return 0.25 * up + 0.5 * c + 0.25 * dn

        def blk(b):
            return pl.ds(pl.multiple_of(b * SUB, SUB), SUB)

        def compute(b0, b1):
            def step(b, carry):
                p, c = carry
                nx = xb[blk(b + 2), :]
                ob[blk(b), :] = stencil(p, c, nx)
                return c, nx
            lax.fori_loop(b0, b1, step, (xb[pl.ds(b0 * SUB, SUB), :], xb[pl.ds((b0 + 1) * SUB, SUB), :]))

        def write(r0, j):
            src = ob.at[pl.ds(r0, half)].reshape(half // STRIDE, STRIDE, n)
            dst = o_hbm.at[pl.ds(r0, half)].reshape(half // STRIDE, STRIDE, n)
            return pltpu.make_async_copy(src.at[:, blk(j)], dst.at[:, blk(j)], sem.at[1])

        groups = STRIDE // SUB
        rd_a.wait()
        rd_c = read(m - TAIL, TAIL, 0)
        rd_c.start()
        compute(1, half // SUB - 1)
        rd_b.wait()

        @pl.loop(1, groups - 1)
        def _(j):
            write(0, j).start()

        rd_c.wait()
        pl.semaphore_wait(bar, has_l.astype(jnp.int32) + has_r.astype(jnp.int32))

        def send(src0, dst0, k, dev):
            return pltpu.make_async_remote_copy(
                xb.at[pl.ds(src0, SUB)], xb.at[pl.ds(dst0, SUB)], sem.at[0], halo_sem.at[k],
                device_id=(dev,), device_id_type=pl.DeviceIdType.MESH)

        to_l, to_r = send(SUB, m + SUB, 1, me - 1), send(m, 0, 0, me + 1)

        @pl.when(has_l)
        def _():
            to_l.start()

        @pl.when(has_r)
        def _():
            to_r.start()

        compute(half // SUB - 1, m // SUB - 1)
        write(0, groups - 1).start()

        @pl.loop(0, groups - 1)
        def _(j):
            write(half, j).start()

        @pl.when(has_l)
        def _():
            to_r.wait_recv()
            ob[0:SUB, :] = stencil(xb[0:SUB, :], xb[SUB:2 * SUB, :], xb[2 * SUB:3 * SUB, :])

        @pl.when(jnp.logical_not(has_l))
        def _():
            c = xb[SUB:2 * SUB, :]
            ob[0:SUB, :] = jnp.where(sub == 0, c, stencil(c, c, xb[2 * SUB:3 * SUB, :]))

        write(0, 0).start()

        @pl.when(has_r)
        def _():
            to_l.wait_recv()
            ob[m - SUB:m, :] = stencil(xb[m - SUB:m, :], xb[m:m + SUB, :], xb[m + SUB:m + 2 * SUB, :])

        @pl.when(jnp.logical_not(has_r))
        def _():
            c = xb[m:m + SUB, :]
            ob[m - SUB:m, :] = jnp.where(sub == SUB - 1, c, stencil(xb[m - SUB:m, :], c, c))

        write(half, groups - 1).start()

        @pl.when(has_l)
        def _():
            to_l.wait_send()

        @pl.when(has_r)
        def _():
            to_r.wait_send()

        pltpu.make_async_copy(ob, o_hbm, sem.at[1]).wait()

    return pl.pallas_call(
        body,
        out_shape=jax.ShapeDtypeStruct((m, n), x.dtype),
        in_specs=[pl.BlockSpec(memory_space=pl.ANY)],
        out_specs=pl.BlockSpec(memory_space=pl.ANY),
        scratch_shapes=[
            pltpu.VMEM((m + 2 * SUB, n), x.dtype),
            pltpu.VMEM((m, n), x.dtype),
            pltpu.SemaphoreType.DMA((2,)),
            pltpu.SemaphoreType.DMA((2,)),
        ],
        compiler_params=pltpu.CompilerParams(collective_id=0, vmem_limit_bytes=100 * 2**20),
    )(x)
```

```python
import jax
import jax.numpy as jnp
from jax import lax
from jax.experimental import pallas as pl
from jax.experimental.pallas import tpu as pltpu

AXIS = "i"
SUB = 8
CHUNKS = (2048, 2048, 2560, 1024, 336, 112, 40, 16)
READ_SEMS = 4
UNROLL = 8
GROUPS = 64


def pallas_dist_halo_stencil_i_m8192_n1024_kernel(x: jax.Array):
    m, n = x.shape
    assert sum(CHUNKS) == m - SUB
    nb = m // SUB
    half = nb // 2
    starts = [sum(CHUNKS[:k]) for k in range(len(CHUNKS) + 1)]

    def body(x_hbm, top, bottom, xb, read_sem, halo_sem):
        def load(r0, rows, s):
            return pltpu.make_async_copy(
                x_hbm.at[pl.ds(r0, rows)], xb.at[pl.ds(SUB + r0, rows)], read_sem.at[s])

        def read(k):
            return load(starts[k], CHUNKS[k], k % READ_SEMS)

        read(0).start()
        load(m - SUB, SUB, 0).start()
        for k in range(1, READ_SEMS):
            read(k).start()

        me = lax.axis_index(AXIS)
        has_l, has_r = me > 0, me < lax.axis_size(AXIS) - 1
        barrier = pltpu.get_barrier_semaphore()

        @pl.when(has_l)
        def _():
            pl.semaphore_signal(barrier, 1, device_id=(me - 1,), device_id_type=pl.DeviceIdType.MESH)

        @pl.when(has_r)
        def _():
            pl.semaphore_signal(barrier, 1, device_id=(me + 1,), device_id_type=pl.DeviceIdType.MESH)

        sub = lax.broadcasted_iota(jnp.int32, (SUB, n), 0)
        outs = [top.reshape(half * SUB, n), bottom.reshape(half * SUB, n)]

        def stencil(p, c, nx):
            up = pltpu.roll(jnp.where(sub == SUB - 1, p, c), 1, 0)
            dn = pltpu.roll(jnp.where(sub == 0, nx, c), SUB - 1, 0)
            return 0.25 * up + 0.5 * c + 0.25 * dn

        def blk(b):
            return pl.ds(b * SUB if isinstance(b, int) else pl.multiple_of(b * SUB, SUB), SUB)

        def compute(b0, b1):
            for h in range(2):
                lo, hi = max(b0, h * half), min(b1, (h + 1) * half)
                if lo >= hi:
                    continue

                def run(b, count, carry, h=h):
                    p, c = carry
                    for u in range(count):
                        nx = xb[blk(b + u + 2), :]
                        outs[h][blk(b + u - h * half), :] = stencil(p, c, nx)
                        p, c = c, nx
                    return p, c

                carry = (xb[blk(lo), :], xb[blk(lo + 1), :])
                trips, rem = divmod(hi - lo, UNROLL)
                if trips > 1:
                    carry = lax.fori_loop(
                        0, trips, lambda t, cr: run(lo + t * UNROLL, UNROLL, cr), carry)
                elif trips == 1:
                    carry = run(lo, UNROLL, carry)
                run(lo + trips * UNROLL, rem, carry)

        def send(src0, dst0, k, dev):
            return pltpu.make_async_remote_copy(
                xb.at[pl.ds(src0, SUB)], xb.at[pl.ds(dst0, SUB)], halo_sem.at[2], halo_sem.at[k],
                device_id=(dev,), device_id_type=pl.DeviceIdType.MESH)

        to_l, to_r = send(SUB, m + SUB, 1, me - 1), send(m, 0, 0, me + 1)

        done = 1
        for k in range(len(CHUNKS)):
            read(k).wait()
            if k == 0:
                load(m - SUB, SUB, 0).wait()
            if k + READ_SEMS < len(CHUNKS):
                read(k + READ_SEMS).start()
            if k == 0:
                pl.semaphore_wait(barrier, has_l.astype(jnp.int32) + has_r.astype(jnp.int32))

                @pl.when(has_l)
                def _():
                    to_l.start()

                @pl.when(has_r)
                def _():
                    to_r.start()

            end = nb - 1 if k == len(CHUNKS) - 1 else starts[k + 1] // SUB - 1
            compute(done, end)
            done = end
            if k == 2:
                @pl.when(has_l)
                def _():
                    to_l.wait_send()
                    to_r.wait_recv()

                @pl.when(jnp.logical_not(has_l))
                def _():
                    xb[blk(0), :] = jnp.zeros((SUB, n), xb.dtype)

                @pl.when(has_r)
                def _():
                    to_r.wait_send()
                    to_l.wait_recv()

                @pl.when(jnp.logical_not(has_r))
                def _():
                    xb[blk(nb + 1), :] = jnp.zeros((SUB, n), xb.dtype)

                c = xb[blk(1), :]
                outs[0][blk(0), :] = jnp.where(
                    sub == jnp.where(has_l, -1, 0), c, stencil(xb[blk(0), :], c, xb[blk(2), :]))

        c = xb[blk(nb), :]
        outs[1][blk(half - 1), :] = jnp.where(
            sub == jnp.where(has_r, -1, SUB - 1), c, stencil(xb[blk(nb - 1), :], c, xb[blk(nb + 1), :]))

    part = jax.ShapeDtypeStruct((GROUPS // 2, m // GROUPS, n), x.dtype)
    parts = pl.pallas_call(
        body,
        out_shape=[part, part],
        in_specs=[pl.BlockSpec(memory_space=pl.ANY)],
        out_specs=[pl.BlockSpec(memory_space=pltpu.VMEM)] * 2,
        scratch_shapes=[
            pltpu.VMEM((m + 2 * SUB, n), x.dtype),
            pltpu.SemaphoreType.DMA((READ_SEMS,)),
            pltpu.SemaphoreType.DMA((3,)),
        ],
        compiler_params=pltpu.CompilerParams(collective_id=0, vmem_limit_bytes=72 * 2**20),
    )(x)
    return jnp.concatenate(parts, axis=0).reshape(m, n)
```

```python
import itertools

import jax
import jax.numpy as jnp
from jax import lax
from jax.experimental import pallas as pl
from jax.experimental.pallas import tpu as pltpu

AXIS = "i"
SUB = 8
UNROLL = 8

STRIDE = 128
SECTIONS = (1408, 1408, 1408, 1408, 896, 640)
DETOURS = (88, 88, 64)
TAIL = (400, 224, 88, 40, 16)
LAST_DETOUR_BEFORE = 3
SEND_AT, RECEIVE_AT = 1, 4

GROUPS, ROW_PARTS, COL_PARTS = 32, 4, 2


def pallas_dist_halo_stencil_i_m8192_n1024_kernel(x: jax.Array):
    m, n = x.shape
    part_rows, part_cols = m // ROW_PARTS, n // COL_PARTS

    section_at = list(itertools.accumulate(SECTIONS, initial=SUB))
    detour_at = list(itertools.accumulate(DETOURS[:-1], initial=section_at[-1]))
    row = tail_start = detour_at.pop()
    tail_at = []
    for i, rows in enumerate(TAIL):
        if i == LAST_DETOUR_BEFORE:
            detour_at.append(row)
            row += DETOURS[-1]
        tail_at.append(row)
        row += rows
    assert row == m - SUB

    def body(x_hbm, *refs):
        *parts, xs, halo, smem, sem = refs
        parts = [p.reshape(part_rows, part_cols) for p in parts]

        def tile(r):
            return pl.ds(r if isinstance(r, int) else pl.multiple_of(r, SUB), SUB)

        def load(r, rows, s):
            return pltpu.make_async_copy(
                x_hbm.at[pl.ds(r, rows)], xs.at[pl.ds(SUB + r, rows)], sem.at[s])

        def start_section(k, j):
            r, rows = section_at[k], SECTIONS[k]
            shape = (rows // STRIDE, STRIDE, n)
            src = x_hbm.at[pl.ds(r, rows)].reshape(shape)
            dst = xs.at[pl.ds(SUB + r, rows)].reshape(shape)
            pltpu.make_async_copy(
                src.at[:, tile(j * SUB)], dst.at[:, tile(j * SUB)], sem.at[k % 2]).start()

        def hop(h):
            r, rows = detour_at[h // 2], DETOURS[h // 2]
            stop = smem.at[pl.ds(0, rows)]
            if h % 2 == 0:
                return pltpu.make_async_copy(x_hbm.at[pl.ds(r, rows)], stop, sem.at[2])
            return pltpu.make_async_copy(stop, xs.at[pl.ds(SUB + r, rows)], sem.at[2])

        def tail(i):
            s = (len(SECTIONS) + i) % 2 if i < 2 else i + 1
            return load(tail_at[i], TAIL[i], s)

        start_section(0, 0)
        hop(0).start()
        pl.loop(1, STRIDE // SUB)(lambda j: start_section(0, j))
        load(0, SUB, 0).start()
        load(m - SUB, SUB, 0).start()

        me = lax.axis_index(AXIS)
        has_up, has_down = me > 0, me < lax.axis_size(AXIS) - 1
        barrier = pltpu.get_barrier_semaphore()
        for exists, peer in ((has_up, me - 1), (has_down, me + 1)):
            pl.when(exists)(lambda peer=peer: pl.semaphore_signal(
                barrier, 1, device_id=(peer,), device_id_type=pl.DeviceIdType.MESH))

        pl.loop(0, STRIDE // SUB)(lambda j: start_section(1, j))

        def send(r, slot, peer):
            return pltpu.make_async_remote_copy(
                xs.at[pl.ds(SUB + r, SUB)], halo.at[slot], sem.at[3], sem.at[4 + slot],
                device_id=(peer,), device_id_type=pl.DeviceIdType.MESH)

        send_up, send_down = send(0, 1, me - 1), send(m - SUB, 0, me + 1)

        def store(p, rows, value):
            for c in range(COL_PARTS):
                parts[p * COL_PARTS + c][rows, :] = value[:, c * part_cols:(c + 1) * part_cols]

        sublane = lax.broadcasted_iota(jnp.int32, (SUB, n), 0)

        def terms(r):
            v = xs[tile(r), :]
            quarter = 0.25 * v
            return pltpu.roll(quarter, 1, 0), pltpu.roll(quarter, SUB - 1, 0), 0.5 * v

        def compute(lo, hi):
            for p in range(ROW_PARTS):
                first, end = max(lo, p * part_rows), min(hi, (p + 1) * part_rows)
                if first >= end:
                    continue

                def run(r, tiles, carry, p=p):
                    prev, cur = carry
                    for t in range(tiles):
                        nxt = terms(r + (t + 2) * SUB)
                        above = jnp.where(sublane == 0, prev[0], cur[0])
                        below = jnp.where(sublane == SUB - 1, nxt[1], cur[1])
                        store(p, tile(r - p * part_rows + t * SUB), above + cur[2] + below)
                        prev, cur = cur, nxt
                    return prev, cur

                step = UNROLL * SUB
                trips, left = divmod(end - first, step)
                carry = terms(first), terms(first + SUB)
                if trips > 1:
                    carry = lax.fori_loop(
                        0, trips, lambda i, c: run(first + i * step, UNROLL, c), carry)
                elif trips == 1:
                    carry = run(first, UNROLL, carry)
                run(first + trips * step, left // SUB, carry)

        xs[tile(0), :] = jnp.zeros((SUB, n), xs.dtype)

        done = 0
        for k, rows in enumerate(SECTIONS):
            last = k == len(SECTIONS) - 1
            if k < 2 * len(DETOURS) - 1:
                hop(k).wait()
                hop(k + 1).start()
            load(0, rows + (2 * SUB if k == 0 else 0), k % 2).wait()
            if last:
                for i in range(1, len(TAIL)):
                    tail(i).start()
            if k == SEND_AT:
                pl.semaphore_wait(barrier, has_up.astype(jnp.int32) + has_down.astype(jnp.int32))
                pl.when(has_up)(send_up.start)
                pl.when(has_down)(send_down.start)

            end = (tail_start if last else section_at[k + 1]) - SUB
            compute(done, end)
            done = end

            if k + 2 < len(SECTIONS):
                pl.loop(0, STRIDE // SUB)(lambda j, k=k: start_section(k + 2, j))
            elif not last:
                tail(0).start()

            if k == RECEIVE_AT:
                for exists, copy in ((has_up, send_up), (has_down, send_down)):
                    pl.when(exists)(copy.wait_send)

                @pl.when(has_up)
                def _():
                    send_down.wait_recv()
                    store(0, pl.ds(0, 1), 0.25 * halo[0, SUB - 1:SUB, :]
                          + 0.5 * xs[SUB:SUB + 1, :] + 0.25 * xs[SUB + 1:SUB + 2, :])

                @pl.when(jnp.logical_not(has_up))
                def _():
                    store(0, pl.ds(0, 1), xs[SUB:SUB + 1, :])

                @pl.when(has_down)
                def _():
                    send_up.wait_recv()
                    xs[tile(SUB + m), :] = halo[1]

                @pl.when(jnp.logical_not(has_down))
                def _():
                    xs[tile(SUB + m), :] = jnp.zeros((SUB, n), xs.dtype)

        for i, rows in enumerate(TAIL):
            if i == LAST_DETOUR_BEFORE:
                hop(2 * len(DETOURS) - 1).wait()
                compute(done, tail_at[i] - SUB)
                done = tail_at[i] - SUB
            tail(i).wait()
            end = m if i == len(TAIL) - 1 else tail_at[i] + rows - SUB
            compute(done, end)
            done = end

        @pl.when(jnp.logical_not(has_down))
        def _():
            store(ROW_PARTS - 1, pl.ds(part_rows - 1, 1), xs[SUB + m - 1:SUB + m, :])

    part = jax.ShapeDtypeStruct((GROUPS // ROW_PARTS, m // GROUPS, part_cols), x.dtype)
    parts = pl.pallas_call(
        body,
        out_shape=[part] * (ROW_PARTS * COL_PARTS),
        in_specs=[pl.BlockSpec(memory_space=pl.ANY)],
        out_specs=[pl.BlockSpec(memory_space=pltpu.VMEM)] * (ROW_PARTS * COL_PARTS),
        scratch_shapes=[
            pltpu.VMEM((m + 2 * SUB, n), x.dtype),
            pltpu.VMEM((2, SUB, n), x.dtype),
            pltpu.SMEM((max(DETOURS), n), x.dtype),
            pltpu.SemaphoreType.DMA((6,)),
        ],
        compiler_params=pltpu.CompilerParams(collective_id=0, vmem_limit_bytes=72 * 2**20),
    )(x)
    bands = [
        jnp.concatenate(parts[p * COL_PARTS:(p + 1) * COL_PARTS], axis=2)
        for p in range(ROW_PARTS)
    ]
    return jnp.concatenate(bands, axis=0).reshape(m, n)
```

```python
import itertools

import jax
import jax.numpy as jnp
from jax import lax
from jax.experimental import pallas as pl
from jax.experimental.pallas import tpu as pltpu

AXIS = "i"
SUB = 8
UNROLL = 8

STRIP = 128
STRIDE = 128
SECTIONS = (2048, 1536, 2048, 1024)
DETOURS = (120, 120)
TAIL = (648, 224, 104, 48, 16)
LAST_DETOUR_BEFORE = 2
STRIPS_OUT_AT, STRIPS_BACK_AT = 0, 1

GROUPS, ROW_PARTS, COL_PARTS = 32, 4, 2

UP, DOWN = 0, 1


def pallas_dist_halo_stencil_i_m8192_n1024_kernel(x: jax.Array):
    m, n = x.shape
    part_rows, part_cols = m // ROW_PARTS, n // COL_PARTS

    strip_at = (0, m - STRIP)
    section_at = list(itertools.accumulate(SECTIONS, initial=STRIP))
    detour_at = list(itertools.accumulate(DETOURS[:-1], initial=section_at[-1]))
    row = tail_start = detour_at.pop()
    tail_at = []
    for i, rows in enumerate(TAIL):
        if i == LAST_DETOUR_BEFORE:
            detour_at.append(row)
            row += DETOURS[-1]
        tail_at.append(row)
        row += rows
    assert row == strip_at[DOWN], "the read schedule must cover the shard"

    def body(x_hbm, *refs):
        *parts, xs, relay, smem, read_sem, hop_sem, send_sem, out_sem, back_sem = refs
        parts = [p.reshape(part_rows, part_cols) for p in parts]

        def tile(r):
            return pl.ds(r if isinstance(r, int) else pl.multiple_of(r, SUB), SUB)

        def staged(r, rows):
            return xs.at[pl.ds(SUB + r, rows)]

        def load(r, rows, sem):
            return pltpu.make_async_copy(x_hbm.at[pl.ds(r, rows)], staged(r, rows), sem)

        def start_section(k, j):
            r, rows = section_at[k], SECTIONS[k]
            shape = (rows // STRIDE, STRIDE, n)
            src = x_hbm.at[pl.ds(r, rows)].reshape(shape)
            dst = staged(r, rows).reshape(shape)
            pltpu.make_async_copy(
                src.at[:, tile(j * SUB)], dst.at[:, tile(j * SUB)], read_sem.at[k % 2]).start()

        def hop(h):
            r, rows = detour_at[h // 2], DETOURS[h // 2]
            stop = smem.at[pl.ds(0, rows)]
            if h % 2 == 0:
                return pltpu.make_async_copy(x_hbm.at[pl.ds(r, rows)], stop, hop_sem)
            return pltpu.make_async_copy(stop, staged(r, rows), hop_sem)

        def tail(i):
            k = len(SECTIONS)
            sems = (read_sem.at[k % 2], read_sem.at[(k + 1) % 2],
                    out_sem.at[UP], out_sem.at[DOWN], send_sem.at[UP])
            return load(tail_at[i], TAIL[i], sems[i])

        start_section(0, 0)
        hop(0).start()
        pl.loop(1, STRIDE // SUB)(lambda j: start_section(0, j))

        me, chips = lax.axis_index(AXIS), lax.axis_size(AXIS)
        peers = (lax.rem(me + chips - 1, chips), lax.rem(me + 1, chips))
        barrier = pltpu.get_barrier_semaphore()
        for peer in peers:
            pl.semaphore_signal(
                barrier, 1, device_id=(peer,), device_id_type=pl.DeviceIdType.MESH)

        pl.loop(0, STRIDE // SUB)(lambda j: start_section(1, j))

        def strip_out(side):
            return pltpu.make_async_remote_copy(
                x_hbm.at[pl.ds(strip_at[side], STRIP)], relay.at[side],
                send_sem.at[side], out_sem.at[side],
                device_id=(peers[side],), device_id_type=pl.DeviceIdType.MESH)

        def strip_back(side):
            return pltpu.make_async_remote_copy(
                relay.at[side], staged(strip_at[side], STRIP),
                send_sem.at[side], back_sem.at[side],
                device_id=(peers[1 - side],), device_id_type=pl.DeviceIdType.MESH)

        def store(p, rows, value):
            for c in range(COL_PARTS):
                parts[p * COL_PARTS + c][rows, :] = value[:, c * part_cols:(c + 1) * part_cols]

        sublane = lax.broadcasted_iota(jnp.int32, (SUB, n), 0)

        def terms(r):
            v = xs[tile(r), :]
            quarter = 0.25 * v
            return pltpu.roll(quarter, 1, 0), pltpu.roll(quarter, SUB - 1, 0), 0.5 * v

        def compute(lo, hi):
            for p in range(ROW_PARTS):
                first, end = max(lo, p * part_rows), min(hi, (p + 1) * part_rows)
                if first >= end:
                    continue

                def run(r, tiles, carry):
                    prev, cur = carry
                    for t in range(tiles):
                        nxt = terms(r + (t + 2) * SUB)
                        above = jnp.where(sublane == 0, prev[0], cur[0])
                        below = jnp.where(sublane == SUB - 1, nxt[1], cur[1])
                        store(p, tile(r - p * part_rows + t * SUB), above + cur[2] + below)
                        prev, cur = cur, nxt
                    return prev, cur

                step = UNROLL * SUB
                trips, left = divmod(end - first, step)
                carry = terms(first), terms(first + SUB)
                if trips > 1:
                    carry = lax.fori_loop(
                        0, trips, lambda i, c: run(first + i * step, UNROLL, c), carry)
                elif trips == 1:
                    carry = run(first, UNROLL, carry)
                run(first + trips * step, left // SUB, carry)

        done = STRIP + SUB
        for k, rows in enumerate(SECTIONS):
            last = k == len(SECTIONS) - 1
            if k < 2 * len(DETOURS) - 1:
                hop(k).wait()
                hop(k + 1).start()
            if k == STRIPS_OUT_AT:
                pl.semaphore_wait(barrier, 2)
                for side in (UP, DOWN):
                    strip_out(side).start()

            load(section_at[k], rows, read_sem.at[k % 2]).wait()
            if last:
                tail(1).start()
            end = (tail_start if last else section_at[k + 1]) - SUB
            compute(done, end)
            done = end
            if k + 2 < len(SECTIONS):
                pl.loop(0, STRIDE // SUB)(lambda j: start_section(k + 2, j))
            elif not last:
                tail(0).start()

            if k == STRIPS_BACK_AT:
                for side in (UP, DOWN):
                    strip_out(side).wait()
                    strip_back(side).start()

        for side in (UP, DOWN):
            strip_back(side).wait()
        for i in range(2, len(TAIL)):
            tail(i).start()

        xs[tile(0), :] = relay[DOWN, STRIP - SUB:STRIP, :]
        xs[tile(SUB + m), :] = relay[UP, 0:SUB, :]
        compute(0, STRIP + SUB)
        compute(strip_at[DOWN] + SUB, m)

        @pl.when(me == 0)
        def _():
            store(0, pl.ds(0, 1), xs[SUB:SUB + 1, :])

        @pl.when(me == chips - 1)
        def _():
            store(ROW_PARTS - 1, pl.ds(part_rows - 1, 1), xs[SUB + m - 1:SUB + m, :])

        for i, rows in enumerate(TAIL):
            if i == LAST_DETOUR_BEFORE:
                hop(2 * len(DETOURS) - 1).wait()
                compute(done, tail_at[i] - SUB)
                done = tail_at[i] - SUB
            tail(i).wait()
            end = tail_at[i] + rows + (SUB if i == len(TAIL) - 1 else -SUB)
            compute(done, end)
            done = end

    part = jax.ShapeDtypeStruct((GROUPS // ROW_PARTS, m // GROUPS, part_cols), x.dtype)
    parts = pl.pallas_call(
        body,
        out_shape=[part] * (ROW_PARTS * COL_PARTS),
        in_specs=[pl.BlockSpec(memory_space=pl.ANY)],
        out_specs=[pl.BlockSpec(memory_space=pltpu.VMEM)] * (ROW_PARTS * COL_PARTS),
        scratch_shapes=[
            pltpu.VMEM((m + 2 * SUB, n), x.dtype),
            pltpu.VMEM((2, STRIP, n), x.dtype),
            pltpu.SMEM((max(DETOURS), n), x.dtype),
            pltpu.SemaphoreType.DMA((2,)),
            pltpu.SemaphoreType.DMA,
            pltpu.SemaphoreType.DMA((2,)),
            pltpu.SemaphoreType.DMA((2,)),
            pltpu.SemaphoreType.DMA((2,)),
        ],
        compiler_params=pltpu.CompilerParams(collective_id=0, vmem_limit_bytes=72 * 2**20),
    )(x)
    bands = [
        jnp.concatenate(parts[p * COL_PARTS:(p + 1) * COL_PARTS], axis=2)
        for p in range(ROW_PARTS)
    ]
    return jnp.concatenate(bands, axis=0).reshape(m, n)
```

```python
import itertools

import jax
import jax.numpy as jnp
from jax import lax
from jax.experimental import pallas as pl
from jax.experimental.pallas import tpu as pltpu

AXIS = "i"
SUB = 8
BAND = 128
UNROLL = 8

EDGES_OUT_AT, EDGES_BACK_AT = 0, 1
SECTIONS = (16, 12, 16, 8)
DETOURS = (120, 120)
TAIL = (456, 320, 168, 72, 24)
LAST_DETOUR_BEFORE = 2

GROUPS, ROW_PARTS, COL_PARTS = 32, 4, 2

UP, DOWN = 0, 1


def _split(r, size):
    if isinstance(r, int):
        return divmod(r, size)
    return lax.div(r, size), pl.multiple_of(lax.rem(r, size), SUB)


def pallas_dist_halo_stencil_i_m8192_n1024_kernel(x: jax.Array):
    m, n = x.shape
    bands = m // BAND
    step = UNROLL * SUB
    group_rows, part_rows, part_cols = m // GROUPS, m // ROW_PARTS, n // COL_PARTS

    section_at = list(itertools.accumulate(SECTIONS, initial=1))
    detour_at = list(itertools.accumulate(DETOURS[:-1], initial=section_at[-1] * BAND))
    row = tail_start = detour_at.pop()
    tail_at = []
    for i, rows in enumerate(TAIL):
        if i == LAST_DETOUR_BEFORE:
            detour_at.append(row)
            row += DETOURS[-1]
        tail_at.append(row)
        row += rows
    assert row == m - BAND, "the read schedule must cover the shard"

    def body(x_hbm, *refs):
        *parts, xs, smem, read_sem, hop_sem, send_sem, out_sem, back_sem = refs

        def start_section(k, j):
            b, count = section_at[k], SECTIONS[k]
            rows = pl.ds(j * SUB if isinstance(j, int) else pl.multiple_of(j * SUB, SUB), SUB)
            pltpu.make_async_copy(
                x_hbm.at[pl.ds(b, count), rows], xs.at[pl.ds(1 + b, count), rows],
                read_sem.at[k % 2]).start()

        def wait_section(k):
            b, count = section_at[k], SECTIONS[k]
            pltpu.make_async_copy(
                x_hbm.at[pl.ds(b, count)], xs.at[pl.ds(1 + b, count)], read_sem.at[k % 2]).wait()

        def hop(h):
            b, r = divmod(detour_at[h // 2], BAND)
            rows = DETOURS[h // 2]
            stop = smem.at[pl.ds(0, rows)]
            if h % 2 == 0:
                return pltpu.make_async_copy(x_hbm.at[b, pl.ds(r, rows)], stop, hop_sem)
            return pltpu.make_async_copy(stop, xs.at[1 + b, pl.ds(r, rows)], hop_sem)

        def tail(i):
            k = len(SECTIONS)
            sem = (read_sem.at[k % 2], read_sem.at[(k + 1) % 2],
                   out_sem.at[UP], out_sem.at[DOWN], send_sem.at[UP])[i]
            copies, row, end = [], tail_at[i], tail_at[i] + TAIL[i]
            while row < end:
                b, r = divmod(row, BAND)
                count = max((end - row) // BAND, 1) if r == 0 else 1
                rows = min(BAND - r, end - row)
                copies.append(pltpu.make_async_copy(
                    x_hbm.at[pl.ds(b, count), pl.ds(r, rows)],
                    xs.at[pl.ds(1 + b, count), pl.ds(r, rows)], sem))
                row += count * rows
            return copies

        def start_tail(i):
            for copy in tail(i):
                copy.start()

        start_section(0, 0)
        hop(0).start()
        pl.loop(1, BAND // SUB)(lambda j: start_section(0, j))

        me, chips = lax.axis_index(AXIS), lax.axis_size(AXIS)
        peers = (lax.rem(me + chips - 1, chips), lax.rem(me + 1, chips))
        barrier = pltpu.get_barrier_semaphore()
        for peer in peers:
            pl.semaphore_signal(
                barrier, 1, device_id=(peer,), device_id_type=pl.DeviceIdType.MESH)

        pl.loop(0, BAND // SUB)(lambda j: start_section(1, j))

        def edge_out(side):
            band, slot = ((0, bands + 1), (bands - 1, 0))[side]
            return pltpu.make_async_remote_copy(
                x_hbm.at[band], xs.at[slot], send_sem.at[side], out_sem.at[side],
                device_id=(peers[side],), device_id_type=pl.DeviceIdType.MESH)

        def edge_back(side):
            band, slot = ((0, bands + 1), (bands - 1, 0))[side]
            return pltpu.make_async_remote_copy(
                xs.at[slot], xs.at[1 + band], send_sem.at[side], back_sem.at[side],
                device_id=(peers[1 - side],), device_id_type=pl.DeviceIdType.MESH)

        def store(p, group, rows, value):
            for c in range(COL_PARTS):
                parts[p * COL_PARTS + c][group, rows, :] = (
                    value[:, c * part_cols:(c + 1) * part_cols])

        sublane = lax.broadcasted_iota(jnp.int32, (SUB, n), 0)

        def terms(row):
            b, r = _split(row + BAND, BAND)
            v = xs[b, pl.ds(r, SUB), :]
            quarter = 0.25 * v
            return pltpu.roll(quarter, 1, 0), pltpu.roll(quarter, SUB - 1, 0), 0.5 * v

        def compute(lo, hi):
            for p in range(ROW_PARTS):
                first, end = max(lo, p * part_rows), min(hi, (p + 1) * part_rows)
                if first >= end:
                    continue

                def run(row, tiles, carry):
                    prev, cur = carry
                    for t in range(tiles):
                        nxt = terms(row + (t + 1) * SUB)
                        above = jnp.where(sublane == 0, prev[0], cur[0])
                        below = jnp.where(sublane == SUB - 1, nxt[1], cur[1])
                        group, r = _split(row - p * part_rows + t * SUB, group_rows)
                        store(p, group, pl.ds(r, SUB), above + cur[2] + below)
                        prev, cur = cur, nxt
                    return prev, cur

                trips, left = divmod(end - first, step)
                carry = terms(first - SUB), terms(first)
                if trips > 1:
                    carry = lax.fori_loop(
                        0, trips, lambda i, c: run(first + i * step, UNROLL, c), carry)
                elif trips == 1:
                    carry = run(first, UNROLL, carry)
                run(first + trips * step, left // SUB, carry)

        done = BAND + SUB
        for k in range(len(SECTIONS)):
            last = k == len(SECTIONS) - 1
            if k < 2 * len(DETOURS) - 1:
                hop(k).wait()
                hop(k + 1).start()
            if k == EDGES_OUT_AT:
                pl.semaphore_wait(barrier, 2)
                for side in (UP, DOWN):
                    edge_out(side).start()

            wait_section(k)
            if last:
                start_tail(1)
            end = ((tail_start if last else section_at[k + 1] * BAND) - SUB) // step * step
            compute(done, end)
            done = end
            if k + 2 < len(SECTIONS):
                pl.loop(0, BAND // SUB)(lambda j: start_section(k + 2, j))
            elif not last:
                start_tail(0)

            if k == EDGES_BACK_AT:
                for side in (UP, DOWN):
                    edge_out(side).wait()
                    edge_back(side).start()

        for side in (UP, DOWN):
            edge_back(side).wait()
        for i in range(2, len(TAIL)):
            start_tail(i)
        compute(0, BAND + SUB)
        compute(m - BAND + SUB, m)

        @pl.when(me == 0)
        def _():
            store(0, 0, pl.ds(0, 1), xs[1, 0:1, :])

        @pl.when(me == chips - 1)
        def _():
            store(ROW_PARTS - 1, GROUPS // ROW_PARTS - 1, pl.ds(group_rows - 1, 1),
                  xs[bands, BAND - 1:BAND, :])

        for i, rows in enumerate(TAIL):
            if i == LAST_DETOUR_BEFORE:
                hop(2 * len(DETOURS) - 1).wait()
                compute(done, tail_at[i] - SUB)
                done = tail_at[i] - SUB
            for copy in tail(i):
                copy.wait()
            end = tail_at[i] + rows + (SUB if i == len(TAIL) - 1 else -SUB)
            compute(done, end)
            done = end

    part = jax.ShapeDtypeStruct((GROUPS // ROW_PARTS, group_rows, part_cols), x.dtype)
    parts = pl.pallas_call(
        body,
        out_shape=[part] * (ROW_PARTS * COL_PARTS),
        in_specs=[pl.BlockSpec(memory_space=pl.ANY)],
        out_specs=[pl.BlockSpec(memory_space=pltpu.VMEM)] * (ROW_PARTS * COL_PARTS),
        scratch_shapes=[
            pltpu.VMEM((bands + 2, BAND, n), x.dtype),
            pltpu.SMEM((max(DETOURS), n), x.dtype),
            pltpu.SemaphoreType.DMA((2,)),
            pltpu.SemaphoreType.DMA,
            pltpu.SemaphoreType.DMA((2,)),
            pltpu.SemaphoreType.DMA((2,)),
            pltpu.SemaphoreType.DMA((2,)),
        ],
        compiler_params=pltpu.CompilerParams(collective_id=0, vmem_limit_bytes=72 * 2**20),
    )(x.reshape(bands, BAND, n))
    rows = [
        jnp.concatenate(parts[p * COL_PARTS:(p + 1) * COL_PARTS], axis=2)
        for p in range(ROW_PARTS)
    ]
    return jnp.concatenate(rows, axis=0).reshape(m, n)
```
